```python
import numpy as np

kernel_name = "dist_moe_cap_ep_outshard_n2048_d512_e8_h1024"

def setup_inputs():
    x = np.random.randn(2048, 512).astype(np.float32)
    router_W = np.random.randn(512, 32).astype(np.float32) * 0.1
    scores64 = x.astype(np.float64) @ router_W.astype(np.float64)
    route_idx = np.argsort(-scores64, axis=-1)[:, :1].astype(np.int32)
    expert_W = np.random.randn(32, 512, 1024).astype(np.float32) * 0.02
    return {"x": x, "router_W": router_W, "route_idx": route_idx, "expert_W": expert_W}

def reference(x, router_W, route_idx, expert_W):
    counts = np.zeros(32, dtype=np.int64)
    out = np.zeros((2048, 1024), dtype=np.float32)
    for i in range(2048):
        e = int(route_idx[i, 0])
        if counts[e] < 51:
            out[i] = x[i] @ expert_W[e]
            counts[e] += 1
    return out
```

```python
import jax
import jax.numpy as jnp
from jax import lax
from jax.experimental import pallas as pl
from jax.experimental.pallas import tpu as pltpu

NT, D, H = 2048, 512, 1024
NE, EL, CAP, ND = 32, 8, 51, 4
TL = NT // ND
CP = 56
NS = EL * CP
HI = 0xFFFF0000
SC = False
NA = 512
LA = NA // 2
LB = (H - NA) // 2


def _bf16_bits(v):
    return pltpu.bitcast(v.astype(jnp.bfloat16).astype(jnp.float32), jnp.uint32)


def _pack(a, b):
    return _bf16_bits(a) | (_bf16_bits(b) >> 16)


def _unpack_hi(p):
    return pltpu.bitcast(p & jnp.uint32(HI), jnp.float32)


def _unpack_lo(p):
    return pltpu.bitcast(p << 16, jnp.float32)


def _dot(a, b):
    return jnp.dot(a, b, preferred_element_type=jnp.float32)


def _dot_nt(a, b):
    return lax.dot_general(a, b, (((1,), (1,)), ((), ())), preferred_element_type=jnp.float32)


class _Scope:
    def __init__(self): self.c = None
    def __call__(self, name):
        if not SC: return
        if self.c is not None: self.c.__exit__(None, None, None)
        self.c = None
        if name:
            self.c = jax.named_scope(name); self.c.__enter__()


def pallas_dist_moe_cap_ep_outshard_n2048_d512_e8_h1024_kernel(x, router_W, route_idx, expert_W):
    del router_W
    r2 = route_idx.reshape(16, 128)

    def body(x_hbm, r_hbm, w_hbm, out_hbm,
             wbuf, xloc, xpack, xg, ysend, ybuf, obuf, rbuf, meta_v, meta_s, zsrc, xdum, ydum,
             wsem, lsem, xr_sem, xs_sem, yr_sem, ys_sem, osem, bar2):
        me = lax.axis_index("i")
        bf = jnp.bfloat16
        sc = _Scope()

        sc('init')
        r_cp = pltpu.make_async_copy(r_hbm, rbuf, lsem.at[0]); r_cp.start()
        x_cp = pltpu.make_async_copy(x_hbm.at[pl.ds(pl.multiple_of(me * TL, TL), TL)], xloc, lsem.at[1]); x_cp.start()
        w_cps = [pltpu.make_async_copy(w_hbm.at[e], wbuf.at[e], wsem.at[e]) for e in range(EL - 1)]
        w_cps.append(pltpu.make_async_copy(w_hbm.at[EL - 1, :, pl.ds(0, NA)], wbuf.at[EL - 1, :, pl.ds(0, NA)], wsem.at[EL - 1]))
        w_cps.append(pltpu.make_async_copy(w_hbm.at[EL - 1, :, pl.ds(NA, H - NA)], wbuf.at[EL - 1, :, pl.ds(NA, H - NA)], wsem.at[EL]))
        for c in w_cps:
            c.start(priority=1)
        zsrc[...] = jnp.zeros_like(zsrc)
        ybuf[0:TL, :] = jnp.zeros((TL, H // 2), jnp.uint32)
        meta_v[...] = jnp.zeros_like(meta_v)
        xg[0:NS, :] = jnp.zeros((NS, D // 2), jnp.uint32)
        bar = pltpu.get_barrier_semaphore()
        for k in range(1, ND):
            pl.semaphore_signal(bar, inc=1, device_id=((me + k) % ND,),
                                device_id_type=pl.DeviceIdType.MESH)

        r_cp.wait()
        sc('route')
        r = rbuf[...]
        lane = lax.broadcasted_iota(jnp.int32, (128, 128), 1)
        sub = lax.broadcasted_iota(jnp.int32, (128, 128), 0)
        U = (sub <= lane).astype(bf)
        J = jnp.ones((128, 128), bf)
        ones8 = jnp.ones((8, 128), bf)

        rrep = jnp.concatenate([r] * NE, axis=0)
        qs = lax.broadcasted_iota(jnp.int32, (512, 128), 0)
        Mb = rrep == (qs >> 4)
        M = Mb.astype(bf)
        pin = _dot(M, U)
        tot = _dot(M, J)
        q0 = lax.broadcasted_iota(jnp.int32, (512, 512), 0)
        q1 = lax.broadcasted_iota(jnp.int32, (512, 512), 1)
        T = (((q0 >> 4) == (q1 >> 4)) & (q1 < q0)).astype(bf)
        incl = pin + _dot(T, tot.astype(bf))
        rk = jnp.where(Mb, incl - 1.0, 0.0)
        rank = rk[0:16]
        for e in range(1, NE):
            rank = rank + rk[16 * e:16 * e + 16]
        rank = rank.astype(jnp.int32)
        acc = rank < CAP
        b16 = lax.broadcasted_iota(jnp.int32, (16, 128), 0)
        l16 = lax.broadcasted_iota(jnp.int32, (16, 128), 1)
        tloc = (b16 & 3) * 128 + l16
        jj = r & 7
        code_ok = (r >> 3) | (jj << 2) | ((jj * CP + rank) << 6)
        code_tr = me | (EL << 2) | ((NS + tloc) << 6)
        meta_v[0:16, :] = jnp.where(acc, code_ok, code_tr)
        meta_v[21:22, 0:16] = _dot_nt(ones8, acc.astype(bf)).astype(jnp.int32)[0:1]

        ML = (rrep[0:128] == (sub >> 4) + me * EL).astype(bf)
        pinL = _dot(ML, U)
        totL = _dot(ML, J)
        TLm = (((sub >> 4) == (lane >> 4)) & (lane < sub)).astype(bf)
        inclL = pinL + _dot(TLm, totL.astype(bf))
        totrow = _dot_nt(ones8, ML)
        TLt = (((sub >> 4) == (lane >> 4)) & (sub < lane)).astype(bf)
        offrow = _dot(totrow.astype(bf), TLt)
        js = lax.broadcasted_iota(jnp.int32, (512, 128), 0)
        ql = lax.broadcasted_iota(jnp.int32, (512, 128), 1)
        sf = (js & 63).astype(jnp.float32)
        offb = offrow[0:1, :]
        endb = offb + totrow[0:1, :]
        S = (((js >> 6) == (ql >> 4)) & (offb <= sf) & (sf < endb)).astype(bf)
        G = _dot(S, jnp.minimum(inclL, 64.0).astype(bf))
        cmp = (G <= sf).astype(bf)
        B8 = ((lax.broadcasted_iota(jnp.int32, (8, 128), 1) & 15) * 128).astype(bf)
        tokT = (_dot_nt(ones8, cmp) + _dot_nt(B8, S)).astype(jnp.int32)
        l512 = lax.broadcasted_iota(jnp.int32, (8, 512), 1)
        validT = (_dot_nt(ones8, S) > 0.5) & ((l512 & 63) < CAP)
        ycode_ok = (tokT >> 9) | ((tokT & (TL - 1)) << 6)
        ycode_tr = me | (1 << 2) | ((TL + (l512 >> 6) * CP + (l512 & 63)) << 6)
        ycode = jnp.where(validT, ycode_ok, ycode_tr)
        for k in range(4):
            meta_v[16 + k:17 + k, :] = ycode[0:1, 128 * k:128 * k + 128]
        meta_v[20:21, :] = jnp.minimum(offrow + totrow, float(CAP)).astype(jnp.int32)[0:1]
        m_cp = pltpu.make_async_copy(meta_v, meta_s, lsem.at[2]); m_cp.start()

        sc('xwait')
        x_cp.wait()
        sc('pack')
        xpack[...] = _pack(xloc[:, 0:256], xloc[:, 256:512])
        sc('mwait')
        m_cp.wait()
        sc('bar')
        pl.semaphore_wait(bar, ND - 1)
        for k in range(1, ND):
            pl.semaphore_signal(bar2, inc=1, device_id=((me + k) % ND,),
                                device_id_type=pl.DeviceIdType.MESH)

        sc('disp')
        def disp(t, carry):
            c = meta_s[4 * me + (t >> 7), t & 127]
            pltpu.make_async_remote_copy(
                xpack.at[pl.ds(t, 1), :], xg.at[pl.ds(c >> 6, 1), :], xs_sem, xr_sem.at[(c >> 2) & 15],
                device_id=(c & 3,), device_id_type=pl.DeviceIdType.MESH).start()
            return carry
        lax.fori_loop(0, TL, disp, 0, unroll=8)

        sc('pad')
        def pad_rows(count, nbits, dst, base, width, sem):
            for k in range(nbits):
                n = 1 << k
                @pl.when(((count >> k) & 1) == 1)
                def _(n=n):
                    pltpu.make_async_copy(zsrc.at[pl.ds(0, n), pl.ds(0, width)],
                                          dst.at[pl.ds(base + n, n), :], sem).start()
        nsum = jnp.int32(0)
        for j in range(EL):
            nj = meta_s[20, 16 * j + 15]
            nsum = nsum + nj
            pad_rows(CP - nj, 6, xdum, 1024 + 64 * j, D // 2, xr_sem.at[j])
        nacc = meta_s[21, 4 * me] + meta_s[21, 4 * me + 1] + meta_s[21, 4 * me + 2] + meta_s[21, 4 * me + 3]
        pad_rows(nacc, 10, xdum, 0, D // 2, xr_sem.at[EL])
        pad_rows(TL - nacc, 10, ydum, 0, H // 2, yr_sem.at[0])
        pad_rows(nsum, 9, ydum, 1024, H // 2, yr_sem.at[1])

        def send_rows(j, lo, width):
            def comb(s, carry):
                idx = j * 64 + s
                c = meta_s[16 + (idx >> 7), idx & 127]
                pltpu.make_async_remote_copy(
                    ysend.at[pl.ds(j * CP + s, 1), pl.ds(lo, width)], ybuf.at[pl.ds(c >> 6, 1), pl.ds(lo, width)],
                    ys_sem, yr_sem.at[(c >> 2) & 1],
                    device_id=(c & 3,), device_id_type=pl.DeviceIdType.MESH).start()
                return carry
            lax.fori_loop(0, CP, comb, 0, unroll=8)

        def mm(j, xa, xb, c0, c1):
            return _dot(xa, wbuf[j, 0:256, c0:c1].astype(bf)) + _dot(xb, wbuf[j, 256:512, c0:c1].astype(bf))

        for j in range(EL):
            sc('wx%d' % j)
            slab = xg.at[pl.ds(j * CP, CP), :]
            pltpu.make_async_copy(slab, slab, xr_sem.at[j]).wait()
            sc('ww%d' % j)
            w_cps[j].wait()
            sc('mm%d' % j)
            p = xg[j * CP:(j + 1) * CP, :]
            xa = _unpack_hi(p).astype(bf)
            xb = _unpack_lo(p).astype(bf)
            rows = slice(j * CP, (j + 1) * CP)
            if j < EL - 1:
                y = mm(j, xa, xb, 0, H)
                ysend[rows, 0:LA] = _pack(y[:, 0:LA], y[:, LA:NA])
                ysend[rows, LA:LA + LB] = _pack(y[:, NA:NA + LB], y[:, NA + LB:H])
                sc('comb%d' % j)
                send_rows(j, 0, H // 2)
            else:
                y = mm(j, xa, xb, 0, NA)
                ysend[rows, 0:LA] = _pack(y[:, 0:LA], y[:, LA:NA])
                sc('comb%d' % j)
                send_rows(j, 0, LA)
                sc('wwB')
                w_cps[EL].wait()
                sc('mmB')
                y = mm(j, xa, xb, NA, H)
                ysend[rows, LA:LA + LB] = _pack(y[:, 0:LB], y[:, LB:2 * LB])
                sc('combB')
                send_rows(j, LA, LB)

        sc('wy')
        yb = ybuf.at[pl.ds(0, TL), :]
        pltpu.make_async_copy(yb, yb, yr_sem.at[0]).wait()
        sc('unpack')
        o_cps = []
        NCH = 8
        RC = TL // NCH
        for k in range(NCH):
            rs = slice(RC * k, RC * k + RC)
            p = ybuf[rs, :]
            obuf[rs, 0:LA] = _unpack_hi(p[:, 0:LA])
            obuf[rs, LA:NA] = _unpack_lo(p[:, 0:LA])
            obuf[rs, NA:NA + LB] = _unpack_hi(p[:, LA:LA + LB])
            obuf[rs, NA + LB:H] = _unpack_lo(p[:, LA:LA + LB])
            c = pltpu.make_async_copy(obuf.at[pl.ds(RC * k, RC)], out_hbm.at[pl.ds(RC * k, RC)], osem.at[k])
            c.start()
            o_cps.append(c)

        sc('drain')
        pltpu.make_async_copy(xpack, xpack, xs_sem).wait()
        pltpu.make_async_copy(ysend, ysend, ys_sem).wait()
        xt = xg.at[pl.ds(NS, TL), :]
        pltpu.make_async_copy(xt, xt, xr_sem.at[EL]).wait()
        yt = ybuf.at[pl.ds(TL, NS), :]
        pltpu.make_async_copy(yt, yt, yr_sem.at[1]).wait()
        pl.semaphore_wait(bar2, ND - 1)
        for c in o_cps:
            c.wait()
        sc(None)

    HBM = pltpu.MemorySpace.HBM
    return pl.pallas_call(
        body,
        out_shape=jax.ShapeDtypeStruct((TL, H), jnp.float32),
        in_specs=[pl.BlockSpec(memory_space=HBM)] * 3,
        out_specs=pl.BlockSpec(memory_space=HBM),
        scratch_shapes=[
            pltpu.VMEM((EL, D, H), jnp.float32),
            pltpu.VMEM((TL, D), jnp.float32),
            pltpu.VMEM((TL, D // 2), jnp.uint32),
            pltpu.VMEM((NS + TL, D // 2), jnp.uint32),
            pltpu.VMEM((NS, H // 2), jnp.uint32),
            pltpu.VMEM((TL + NS, H // 2), jnp.uint32),
            pltpu.VMEM((TL, H), jnp.float32),
            pltpu.VMEM((16, 128), jnp.int32),
            pltpu.VMEM((24, 128), jnp.int32),
            pltpu.SMEM((24, 128), jnp.int32),
            pltpu.VMEM((TL, H // 2), jnp.uint32),
            pltpu.VMEM((1024 + 64 * EL, D // 2), jnp.uint32),
            pltpu.VMEM((1024 + 512, H // 2), jnp.uint32),
            pltpu.SemaphoreType.DMA((EL + 1,)),
            pltpu.SemaphoreType.DMA((3,)),
            pltpu.SemaphoreType.DMA((EL + 1,)),
            pltpu.SemaphoreType.DMA,
            pltpu.SemaphoreType.DMA((2,)),
            pltpu.SemaphoreType.DMA,
            pltpu.SemaphoreType.DMA((8,)),
            pltpu.SemaphoreType.REGULAR,
        ],
        compiler_params=pltpu.CompilerParams(collective_id=0, vmem_limit_bytes=64 * 1024 * 1024),
    )(x, r2, expert_W)
```

```python
import jax
import jax.numpy as jnp
from jax import lax
from jax.experimental import pallas as pl
from jax.experimental.pallas import tpu as pltpu

NT, D, H = 2048, 512, 1024
NE, EL, CAP, ND = 32, 8, 51, 4
TL = NT // ND
CP = 56
NS = EL * CP
HH = H // 2
LQ = H // 4
DH = D // 2


def _bf16_bits(v):
    return pltpu.bitcast(v.astype(jnp.bfloat16).astype(jnp.float32), jnp.uint32)


def _pack(a, b):
    return _bf16_bits(a) | (_bf16_bits(b) >> 16)


def _unpack_hi(p):
    return pltpu.bitcast(p & jnp.uint32(0xFFFF0000), jnp.float32)


def _unpack_lo(p):
    return pltpu.bitcast(p << 16, jnp.float32)


def _dot(a, b):
    return jnp.dot(a, b, preferred_element_type=jnp.float32)


def _dot_nt(a, b):
    return lax.dot_general(a, b, (((1,), (1,)), ((), ())), preferred_element_type=jnp.float32)


def pallas_dist_moe_cap_ep_outshard_n2048_d512_e8_h1024_kernel(x, router_W, route_idx, expert_W):
    del router_W
    r2 = route_idx.reshape(16, 128)

    def body(x_hbm, r_hbm, w_hbm, out_ref,
             wbuf, xloc, xpack, xg, ysend, ybuf, rbuf, meta_v, meta_s, zsrc, xdum, ydum, hdum,
             wsem, lsem, xr_sem, xs_sem, yr_sem, ys_sem, bar2):
        me = lax.axis_index("i")
        bf = jnp.bfloat16
        MESH = pl.DeviceIdType.MESH

        r_cp = pltpu.make_async_copy(r_hbm, rbuf, lsem.at[0])
        r_cp.start()
        x_cp = pltpu.make_async_copy(x_hbm.at[pl.ds(pl.multiple_of(me * TL, TL), TL)], xloc, lsem.at[1])
        x_cp.start()
        w_cps = [pltpu.make_async_copy(w_hbm.at[e], wbuf.at[e], wsem.at[e]) for e in range(EL - 1)]
        w_cps.append(pltpu.make_async_copy(w_hbm.at[EL - 1, :, pl.ds(0, HH)],
                                           wbuf.at[EL - 1, :, pl.ds(0, HH)], wsem.at[EL - 1]))
        for kk in range(2):
            w_cps.append(pltpu.make_async_copy(w_hbm.at[EL - 1, pl.ds(DH * kk, DH), pl.ds(HH, HH)],
                                               wbuf.at[EL - 1, pl.ds(DH * kk, DH), pl.ds(HH, HH)],
                                               wsem.at[EL + kk]))
        for c in w_cps:
            c.start(priority=1)

        zsrc[...] = jnp.zeros_like(zsrc)
        ybuf[0:TL, :] = jnp.zeros((TL, HH), jnp.uint32)
        xg[0:NS, :] = jnp.zeros((NS, DH), jnp.uint32)
        meta_v[...] = jnp.zeros_like(meta_v)
        bar = pltpu.get_barrier_semaphore()
        for k in range(1, ND):
            pl.semaphore_signal(bar, inc=1, device_id=((me + k) % ND,), device_id_type=MESH)

        r_cp.wait()
        r = rbuf[...]
        lane = lax.broadcasted_iota(jnp.int32, (128, 128), 1)
        sub = lax.broadcasted_iota(jnp.int32, (128, 128), 0)
        U = (sub <= lane).astype(bf)
        J = jnp.ones((128, 128), bf)
        ones8 = jnp.ones((8, 128), bf)

        rrep = jnp.concatenate([r] * NE, axis=0)
        qs = lax.broadcasted_iota(jnp.int32, (512, 128), 0)
        Mb = rrep == (qs >> 4)
        M = Mb.astype(bf)
        q0 = lax.broadcasted_iota(jnp.int32, (512, 512), 0)
        q1 = lax.broadcasted_iota(jnp.int32, (512, 512), 1)
        T = (((q0 >> 4) == (q1 >> 4)) & (q1 < q0)).astype(bf)
        incl = _dot(M, U) + _dot(T, _dot(M, J).astype(bf))
        rk = jnp.where(Mb, incl - 1.0, 0.0)
        rank = rk[0:16]
        for e in range(1, NE):
            rank = rank + rk[16 * e:16 * e + 16]
        rank = rank.astype(jnp.int32)
        acc = rank < CAP
        b16 = lax.broadcasted_iota(jnp.int32, (16, 128), 0)
        l16 = lax.broadcasted_iota(jnp.int32, (16, 128), 1)
        jj = r & (EL - 1)
        code_ok = (r >> 3) | (jj << 2) | ((jj * CP + rank) << 6)
        code_tr = me | (EL << 2) | ((NS + (b16 & 3) * 128 + l16) << 6)
        meta_v[0:16, :] = jnp.where(acc, code_ok, code_tr)
        meta_v[21:22, 0:16] = _dot_nt(ones8, acc.astype(bf)).astype(jnp.int32)[0:1]
        meta_v[22:23, 0:16] = _dot_nt(ones8, (acc & (jj == EL - 1)).astype(bf)).astype(jnp.int32)[0:1]

        ML = (rrep[0:128] == (sub >> 4) + me * EL).astype(bf)
        TLm = (((sub >> 4) == (lane >> 4)) & (lane < sub)).astype(bf)
        inclL = _dot(ML, U) + _dot(TLm, _dot(ML, J).astype(bf))
        totrow = _dot_nt(ones8, ML)
        TLt = (((sub >> 4) == (lane >> 4)) & (sub < lane)).astype(bf)
        offrow = _dot(totrow.astype(bf), TLt)
        js = lax.broadcasted_iota(jnp.int32, (512, 128), 0)
        ql = lax.broadcasted_iota(jnp.int32, (512, 128), 1)
        sf = (js & 63).astype(jnp.float32)
        offb = offrow[0:1, :]
        endb = offb + totrow[0:1, :]
        S = (((js >> 6) == (ql >> 4)) & (offb <= sf) & (sf < endb)).astype(bf)
        G = _dot(S, jnp.minimum(inclL, 64.0).astype(bf))
        cmp = (G <= sf).astype(bf)
        B8 = ((lax.broadcasted_iota(jnp.int32, (8, 128), 1) & 15) * 128).astype(bf)
        tokT = (_dot_nt(ones8, cmp) + _dot_nt(B8, S)).astype(jnp.int32)
        l512 = lax.broadcasted_iota(jnp.int32, (8, 512), 1)
        validT = (_dot_nt(ones8, S) > 0.5) & ((l512 & 63) < CAP)
        ycode_ok = (tokT >> 9) | ((tokT & (TL - 1)) << 6)
        ycode_tr = me | (1 << 2) | ((TL + (l512 >> 6) * CP + (l512 & 63)) << 6)
        ycode = jnp.where(validT, ycode_ok, ycode_tr)
        for k in range(4):
            meta_v[16 + k:17 + k, :] = ycode[0:1, 128 * k:128 * k + 128]
        meta_v[20:21, :] = jnp.minimum(offrow + totrow, float(CAP)).astype(jnp.int32)[0:1]
        m_cp = pltpu.make_async_copy(meta_v, meta_s, lsem.at[2])
        m_cp.start()

        x_cp.wait()
        xpack[...] = _pack(xloc[:, 0:DH], xloc[:, DH:D])
        m_cp.wait()
        pl.semaphore_wait(bar, ND - 1)
        for k in range(1, ND):
            pl.semaphore_signal(bar2, inc=1, device_id=((me + k) % ND,), device_id_type=MESH)

        def disp(t, carry):
            c = meta_s[4 * me + (t >> 7), t & 127]
            pltpu.make_async_remote_copy(
                xpack.at[pl.ds(t, 1), :], xg.at[pl.ds(c >> 6, 1), :], xs_sem, xr_sem.at[(c >> 2) & 15],
                device_id=(c & 3,), device_id_type=MESH).start()
            return carry
        lax.fori_loop(0, TL, disp, 0, unroll=8)

        def pad_rows(count, nbits, dst, base, width, sem):
            for k in range(nbits):
                n = 1 << k

                @pl.when(((count >> k) & 1) == 1)
                def _(n=n):
                    pltpu.make_async_copy(zsrc.at[pl.ds(0, n), pl.ds(0, width)],
                                          dst.at[pl.ds(base + n, n), :], sem).start()

        nsum = jnp.int32(0)
        for j in range(EL):
            nj = meta_s[20, 16 * j + 15]
            nsum = nsum + nj
            pad_rows(CP - nj, 6, xdum, 1024 + 64 * j, DH, xr_sem.at[j])
        nacc = meta_s[21, 4 * me] + meta_s[21, 4 * me + 1] + meta_s[21, 4 * me + 2] + meta_s[21, 4 * me + 3]
        nlate = meta_s[22, 4 * me] + meta_s[22, 4 * me + 1] + meta_s[22, 4 * me + 2] + meta_s[22, 4 * me + 3]
        pad_rows(nacc, 10, xdum, 0, DH, xr_sem.at[EL])
        pad_rows(TL - nacc, 10, ydum, 0, HH, yr_sem.at[0])
        pad_rows(nlate, 10, hdum, 0, LQ, yr_sem.at[0])
        pad_rows(TL - nlate, 10, hdum, 1024, LQ, yr_sem.at[2])
        pad_rows(nsum, 9, ydum, 1024, HH, yr_sem.at[1])

        def send_rows(j, lo, width, late=False):
            def comb(s, carry):
                idx = j * 64 + s
                c = meta_s[16 + (idx >> 7), idx & 127]
                tr = (c >> 2) & 1
                pltpu.make_async_remote_copy(
                    ysend.at[pl.ds(j * CP + s, 1), pl.ds(lo, width)],
                    ybuf.at[pl.ds(c >> 6, 1), pl.ds(lo, width)],
                    ys_sem, yr_sem.at[(2 - tr) if late else tr],
                    device_id=(c & 3,), device_id_type=MESH).start()
                return carry
            lax.fori_loop(0, CP, comb, 0, unroll=True)

        for j in range(EL):
            slab = xg.at[pl.ds(j * CP, CP), :]
            pltpu.make_async_copy(slab, slab, xr_sem.at[j]).wait()
            w_cps[j].wait()
            p = xg[j * CP:(j + 1) * CP, :]
            xa = _unpack_hi(p).astype(bf)
            xb = _unpack_lo(p).astype(bf)
            rows = slice(j * CP, (j + 1) * CP)
            if j < EL - 1:
                y = _dot(xa, wbuf[j, 0:DH, :].astype(bf)) + _dot(xb, wbuf[j, DH:D, :].astype(bf))
                ysend[rows, 0:LQ] = _pack(y[:, 0:LQ], y[:, LQ:HH])
                ysend[rows, LQ:HH] = _pack(y[:, HH:HH + LQ], y[:, HH + LQ:H])
                send_rows(j, 0, HH)
            else:
                y = _dot(xa, wbuf[j, 0:DH, 0:HH].astype(bf)) + _dot(xb, wbuf[j, DH:D, 0:HH].astype(bf))
                ysend[rows, 0:LQ] = _pack(y[:, 0:LQ], y[:, LQ:HH])
                send_rows(j, 0, LQ)
                w_cps[EL].wait()
                y = _dot(xa, wbuf[j, 0:DH, HH:H].astype(bf))
                w_cps[EL + 1].wait()
                y = y + _dot(xb, wbuf[j, DH:D, HH:H].astype(bf))
                ysend[rows, LQ:HH] = _pack(y[:, 0:LQ], y[:, LQ:HH])
                send_rows(j, LQ, LQ, late=True)

        RC = 64
        yb = ybuf.at[pl.ds(0, TL), :]
        pltpu.make_async_copy(yb, yb, yr_sem.at[0]).wait()
        for k in range(TL // RC):
            rs = slice(RC * k, RC * k + RC)
            p = ybuf[rs, 0:LQ]
            out_ref[rs, 0:LQ] = _unpack_hi(p)
            out_ref[rs, LQ:HH] = _unpack_lo(p)
        yb2 = ybuf.at[pl.ds(0, TL), pl.ds(LQ, LQ)]
        pltpu.make_async_copy(yb2, yb2, yr_sem.at[2]).wait()
        for k in range(TL // RC):
            rs = slice(RC * k, RC * k + RC)
            p = ybuf[rs, LQ:HH]
            out_ref[rs, HH:HH + LQ] = _unpack_hi(p)
            out_ref[rs, HH + LQ:H] = _unpack_lo(p)

        pltpu.make_async_copy(xpack, xpack, xs_sem).wait()
        pltpu.make_async_copy(ysend, ysend, ys_sem).wait()
        xt = xg.at[pl.ds(NS, TL), :]
        pltpu.make_async_copy(xt, xt, xr_sem.at[EL]).wait()
        yt = ybuf.at[pl.ds(TL, NS), :]
        pltpu.make_async_copy(yt, yt, yr_sem.at[1]).wait()
        pl.semaphore_wait(bar2, ND - 1)

    HBM = pltpu.MemorySpace.HBM
    return pl.pallas_call(
        body,
        out_shape=jax.ShapeDtypeStruct((TL, H), jnp.float32),
        in_specs=[pl.BlockSpec(memory_space=HBM)] * 3,
        out_specs=pl.BlockSpec(memory_space=pltpu.VMEM),
        scratch_shapes=[
            pltpu.VMEM((EL, D, H), jnp.float32),
            pltpu.VMEM((TL, D), jnp.float32),
            pltpu.VMEM((TL, DH), jnp.uint32),
            pltpu.VMEM((NS + TL, DH), jnp.uint32),
            pltpu.VMEM((NS, HH), jnp.uint32),
            pltpu.VMEM((TL + NS, HH), jnp.uint32),
            pltpu.VMEM((16, 128), jnp.int32),
            pltpu.VMEM((24, 128), jnp.int32),
            pltpu.SMEM((24, 128), jnp.int32),
            pltpu.VMEM((TL, HH), jnp.uint32),
            pltpu.VMEM((1024 + 64 * EL, DH), jnp.uint32),
            pltpu.VMEM((1024 + 512, HH), jnp.uint32),
            pltpu.VMEM((2048, LQ), jnp.uint32),
            pltpu.SemaphoreType.DMA((EL + 2,)),
            pltpu.SemaphoreType.DMA((3,)),
            pltpu.SemaphoreType.DMA((EL + 1,)),
            pltpu.SemaphoreType.DMA,
            pltpu.SemaphoreType.DMA((3,)),
            pltpu.SemaphoreType.DMA,
            pltpu.SemaphoreType.REGULAR,
        ],
        compiler_params=pltpu.CompilerParams(collective_id=0, vmem_limit_bytes=64 * 1024 * 1024),
    )(x, r2, expert_W)
```

```python
import jax
import jax.numpy as jnp
from jax import lax
from jax.experimental import pallas as pl
from jax.experimental.pallas import tpu as pltpu

NT, D, H = 2048, 512, 1024
NE, EL, CAP, ND = 32, 8, 51, 4
TL = NT // ND
CP = 56
NS = EL * CP
HH = H // 2
LQ = H // 4
DH = D // 2


def _bf16_bits(v):
    return pltpu.bitcast(v.astype(jnp.bfloat16).astype(jnp.float32), jnp.uint32)


def _pack(a, b):
    return _bf16_bits(a) | (_bf16_bits(b) >> 16)


def _unpack_hi(p):
    return pltpu.bitcast(p & jnp.uint32(0xFFFF0000), jnp.float32)


def _unpack_lo(p):
    return pltpu.bitcast(p << 16, jnp.float32)


def _dot(a, b):
    return jnp.dot(a, b, preferred_element_type=jnp.float32)


def _dot_nt(a, b):
    return lax.dot_general(a, b, (((1,), (1,)), ((), ())), preferred_element_type=jnp.float32)


def pallas_dist_moe_cap_ep_outshard_n2048_d512_e8_h1024_kernel(x, router_W, route_idx, expert_W):
    del router_W
    r2 = route_idx.reshape(16, 128)

    def body(x_hbm, r_hbm, w_hbm, out_ref,
             wbuf, xloc, xpack, xg, ysend, ybuf, rbuf, meta_v, meta_s, zsrc, xdum, ydum, hdum, ypart,
             wsem, lsem, xr_sem, xs_sem, yr_sem, ys_sem, bar2):
        me = lax.axis_index("i")
        bf = jnp.bfloat16
        MESH = pl.DeviceIdType.MESH

        r_cp = pltpu.make_async_copy(r_hbm, rbuf, lsem.at[0])
        r_cp.start()
        x_cp = pltpu.make_async_copy(x_hbm.at[pl.ds(pl.multiple_of(me * TL, TL), TL)], xloc, lsem.at[1])
        x_cp.start()
        w_cps = [pltpu.make_async_copy(w_hbm.at[e], wbuf.at[e], wsem.at[e]) for e in range(EL - 1)]
        w_cps.append(pltpu.make_async_copy(w_hbm.at[EL - 1, :, pl.ds(0, HH)],
                                           wbuf.at[EL - 1, :, pl.ds(0, HH)], wsem.at[EL - 1]))
        for kk in range(2):
            w_cps.append(pltpu.make_async_copy(w_hbm.at[EL - 1, pl.ds(DH * kk, DH), pl.ds(HH, HH)],
                                               wbuf.at[EL - 1, pl.ds(DH * kk, DH), pl.ds(HH, HH)],
                                               wsem.at[EL + kk]))
        for c in w_cps:
            c.start(priority=1)

        zsrc[...] = jnp.zeros_like(zsrc)
        ybuf[0:TL, :] = jnp.zeros((TL, HH), jnp.uint32)
        xg[0:NS, :] = jnp.zeros((NS, DH), jnp.uint32)
        meta_v[...] = jnp.zeros_like(meta_v)
        bar = pltpu.get_barrier_semaphore()
        for k in range(1, ND):
            pl.semaphore_signal(bar, inc=1, device_id=((me + k) % ND,), device_id_type=MESH)

        r_cp.wait()
        r = rbuf[...]
        lane = lax.broadcasted_iota(jnp.int32, (128, 128), 1)
        sub = lax.broadcasted_iota(jnp.int32, (128, 128), 0)
        U = (sub <= lane).astype(bf)
        J = jnp.ones((128, 128), bf)
        ones8 = jnp.ones((8, 128), bf)

        rrep = jnp.concatenate([r] * NE, axis=0)
        qs = lax.broadcasted_iota(jnp.int32, (512, 128), 0)
        Mb = rrep == (qs >> 4)
        M = Mb.astype(bf)
        q0 = lax.broadcasted_iota(jnp.int32, (512, 512), 0)
        q1 = lax.broadcasted_iota(jnp.int32, (512, 512), 1)
        T = (((q0 >> 4) == (q1 >> 4)) & (q1 < q0)).astype(bf)
        incl = _dot(M, U) + _dot(T, _dot(M, J).astype(bf))
        rk = jnp.where(Mb, incl - 1.0, 0.0)
        rank = rk[0:16]
        for e in range(1, NE):
            rank = rank + rk[16 * e:16 * e + 16]
        rank = rank.astype(jnp.int32)
        acc = rank < CAP
        b16 = lax.broadcasted_iota(jnp.int32, (16, 128), 0)
        l16 = lax.broadcasted_iota(jnp.int32, (16, 128), 1)
        jj = r & (EL - 1)
        code_ok = (r >> 3) | (jj << 2) | ((jj * CP + rank) << 6)
        code_tr = me | (EL << 2) | ((NS + (b16 & 3) * 128 + l16) << 6)
        meta_v[0:16, :] = jnp.where(acc, code_ok, code_tr)
        meta_v[21:22, 0:16] = _dot_nt(ones8, acc.astype(bf)).astype(jnp.int32)[0:1]
        meta_v[22:23, 0:16] = _dot_nt(ones8, (acc & (jj == EL - 1)).astype(bf)).astype(jnp.int32)[0:1]

        ML = (rrep[0:128] == (sub >> 4) + me * EL).astype(bf)
        TLm = (((sub >> 4) == (lane >> 4)) & (lane < sub)).astype(bf)
        inclL = _dot(ML, U) + _dot(TLm, _dot(ML, J).astype(bf))
        totrow = _dot_nt(ones8, ML)
        TLt = (((sub >> 4) == (lane >> 4)) & (sub < lane)).astype(bf)
        offrow = _dot(totrow.astype(bf), TLt)
        js = lax.broadcasted_iota(jnp.int32, (512, 128), 0)
        ql = lax.broadcasted_iota(jnp.int32, (512, 128), 1)
        sf = (js & 63).astype(jnp.float32)
        offb = offrow[0:1, :]
        endb = offb + totrow[0:1, :]
        S = (((js >> 6) == (ql >> 4)) & (offb <= sf) & (sf < endb)).astype(bf)
        G = _dot(S, jnp.minimum(inclL, 64.0).astype(bf))
        cmp = (G <= sf).astype(bf)
        B8 = ((lax.broadcasted_iota(jnp.int32, (8, 128), 1) & 15) * 128).astype(bf)
        tokT = (_dot_nt(ones8, cmp) + _dot_nt(B8, S)).astype(jnp.int32)
        l512 = lax.broadcasted_iota(jnp.int32, (8, 512), 1)
        validT = (_dot_nt(ones8, S) > 0.5) & ((l512 & 63) < CAP)
        ycode_ok = (tokT >> 9) | ((tokT & (TL - 1)) << 6)
        ycode_tr = me | (1 << 2) | ((TL + (l512 >> 6) * CP + (l512 & 63)) << 6)
        ycode = jnp.where(validT, ycode_ok, ycode_tr)
        for k in range(4):
            meta_v[16 + k:17 + k, :] = ycode[0:1, 128 * k:128 * k + 128]
        meta_v[20:21, :] = jnp.minimum(offrow + totrow, float(CAP)).astype(jnp.int32)[0:1]
        m_cp = pltpu.make_async_copy(meta_v, meta_s, lsem.at[2])
        m_cp.start()

        x_cp.wait()
        xpack[...] = _pack(xloc[:, 0:DH], xloc[:, DH:D])
        m_cp.wait()
        pl.semaphore_wait(bar, ND - 1)
        for k in range(1, ND):
            pl.semaphore_signal(bar2, inc=1, device_id=((me + k) % ND,), device_id_type=MESH)

        def disp(t, carry):
            c = meta_s[4 * me + (t >> 7), t & 127]
            pltpu.make_async_remote_copy(
                xpack.at[pl.ds(t, 1), :], xg.at[pl.ds(c >> 6, 1), :], xs_sem, xr_sem.at[(c >> 2) & 15],
                device_id=(c & 3,), device_id_type=MESH).start()
            return carry
        lax.fori_loop(0, TL, disp, 0, unroll=8)

        def pad_rows(count, nbits, dst, base, width, sem):
            for k in range(nbits):
                n = 1 << k

                @pl.when(((count >> k) & 1) == 1)
                def _(n=n):
                    pltpu.make_async_copy(zsrc.at[pl.ds(0, n), pl.ds(0, width)],
                                          dst.at[pl.ds(base + n, n), :], sem).start()

        nsum = jnp.int32(0)
        for j in range(EL):
            nj = meta_s[20, 16 * j + 15]
            nsum = nsum + nj
            pad_rows(CP - nj, 6, xdum, 1024 + 64 * j, DH, xr_sem.at[j])
        nacc = meta_s[21, 4 * me] + meta_s[21, 4 * me + 1] + meta_s[21, 4 * me + 2] + meta_s[21, 4 * me + 3]
        nlate = meta_s[22, 4 * me] + meta_s[22, 4 * me + 1] + meta_s[22, 4 * me + 2] + meta_s[22, 4 * me + 3]
        pad_rows(nacc, 10, xdum, 0, DH, xr_sem.at[EL])
        pad_rows(TL - nacc, 10, ydum, 0, HH, yr_sem.at[0])
        pad_rows(nlate, 10, hdum, 0, LQ, yr_sem.at[0])
        pad_rows(TL - nlate, 10, hdum, 1024, LQ, yr_sem.at[2])
        pad_rows(nsum, 9, ydum, 1024, HH, yr_sem.at[1])

        def send_rows(j, lo, width, late=False):
            def comb(s, carry):
                idx = j * 64 + s
                c = meta_s[16 + (idx >> 7), idx & 127]
                tr = (c >> 2) & 1
                pltpu.make_async_remote_copy(
                    ysend.at[pl.ds(j * CP + s, 1), pl.ds(lo, width)],
                    ybuf.at[pl.ds(c >> 6, 1), pl.ds(lo, width)],
                    ys_sem, yr_sem.at[(2 - tr) if late else tr],
                    device_id=(c & 3,), device_id_type=MESH).start()
                return carry
            lax.fori_loop(0, CP, comb, 0, unroll=True)

        for j in range(EL):
            slab = xg.at[pl.ds(j * CP, CP), :]
            pltpu.make_async_copy(slab, slab, xr_sem.at[j]).wait()
            w_cps[j].wait()
            p = xg[j * CP:(j + 1) * CP, :]
            xa = _unpack_hi(p).astype(bf)
            xb = _unpack_lo(p).astype(bf)
            rows = slice(j * CP, (j + 1) * CP)
            if j < EL - 1:
                y = _dot(xa, wbuf[j, 0:DH, :].astype(bf)) + _dot(xb, wbuf[j, DH:D, :].astype(bf))
                ysend[rows, 0:LQ] = _pack(y[:, 0:LQ], y[:, LQ:HH])
                ysend[rows, LQ:HH] = _pack(y[:, HH:HH + LQ], y[:, HH + LQ:H])
                send_rows(j, 0, HH)
            else:
                y = _dot(xa, wbuf[j, 0:DH, 0:HH].astype(bf)) + _dot(xb, wbuf[j, DH:D, 0:HH].astype(bf))
                ysend[rows, 0:LQ] = _pack(y[:, 0:LQ], y[:, LQ:HH])
                send_rows(j, 0, LQ)
                w_cps[EL].wait()
                ypart[...] = _dot(xa, wbuf[j, 0:DH, HH:H].astype(bf))
                w_cps[EL + 1].wait()
                y = ypart[...] + _dot(xb, wbuf[j, DH:D, HH:H].astype(bf))
                ysend[rows, LQ:HH] = _pack(y[:, 0:LQ], y[:, LQ:HH])
                send_rows(j, LQ, LQ, late=True)

        RC = 64
        yb = ybuf.at[pl.ds(0, TL), :]
        pltpu.make_async_copy(yb, yb, yr_sem.at[0]).wait()
        for k in range(TL // RC):
            rs = slice(RC * k, RC * k + RC)
            p = ybuf[rs, 0:LQ]
            out_ref[rs, 0:LQ] = _unpack_hi(p)
            out_ref[rs, LQ:HH] = _unpack_lo(p)
        yb2 = ybuf.at[pl.ds(0, TL), pl.ds(LQ, LQ)]
        pltpu.make_async_copy(yb2, yb2, yr_sem.at[2]).wait()
        for k in range(TL // RC):
            rs = slice(RC * k, RC * k + RC)
            p = ybuf[rs, LQ:HH]
            out_ref[rs, HH:HH + LQ] = _unpack_hi(p)
            out_ref[rs, HH + LQ:H] = _unpack_lo(p)

        pltpu.make_async_copy(xpack, xpack, xs_sem).wait()
        pltpu.make_async_copy(ysend, ysend, ys_sem).wait()
        xt = xg.at[pl.ds(NS, TL), :]
        pltpu.make_async_copy(xt, xt, xr_sem.at[EL]).wait()
        yt = ybuf.at[pl.ds(TL, NS), :]
        pltpu.make_async_copy(yt, yt, yr_sem.at[1]).wait()
        pl.semaphore_wait(bar2, ND - 1)

    HBM = pltpu.MemorySpace.HBM
    return pl.pallas_call(
        body,
        out_shape=jax.ShapeDtypeStruct((TL, H), jnp.float32),
        in_specs=[pl.BlockSpec(memory_space=HBM)] * 3,
        out_specs=pl.BlockSpec(memory_space=pltpu.VMEM),
        scratch_shapes=[
            pltpu.VMEM((EL, D, H), jnp.float32),
            pltpu.VMEM((TL, D), jnp.float32),
            pltpu.VMEM((TL, DH), jnp.uint32),
            pltpu.VMEM((NS + TL, DH), jnp.uint32),
            pltpu.VMEM((NS, HH), jnp.uint32),
            pltpu.VMEM((TL + NS, HH), jnp.uint32),
            pltpu.VMEM((16, 128), jnp.int32),
            pltpu.VMEM((24, 128), jnp.int32),
            pltpu.SMEM((24, 128), jnp.int32),
            pltpu.VMEM((TL, HH), jnp.uint32),
            pltpu.VMEM((1024 + 64 * EL, DH), jnp.uint32),
            pltpu.VMEM((1024 + 512, HH), jnp.uint32),
            pltpu.VMEM((2048, LQ), jnp.uint32),
            pltpu.VMEM((CP, HH), jnp.float32),
            pltpu.SemaphoreType.DMA((EL + 2,)),
            pltpu.SemaphoreType.DMA((3,)),
            pltpu.SemaphoreType.DMA((EL + 1,)),
            pltpu.SemaphoreType.DMA,
            pltpu.SemaphoreType.DMA((3,)),
            pltpu.SemaphoreType.DMA,
            pltpu.SemaphoreType.REGULAR,
        ],
        compiler_params=pltpu.CompilerParams(collective_id=0, vmem_limit_bytes=64 * 1024 * 1024),
    )(x, r2, expert_W)
```
